```python
import numpy as np

kernel_name = "dist_layernorm_xy_m6144_n2048"

def setup_inputs():
    x = np.random.randn(12288, 4096).astype(np.float32)
    gamma = np.random.randn(4096).astype(np.float32)
    beta = np.random.randn(4096).astype(np.float32)
    return {"x": x, "gamma": gamma, "beta": beta}

def reference(x: np.ndarray, gamma: np.ndarray, beta: np.ndarray) -> np.ndarray:
    eps = 1e-5
    mean = np.mean(x, axis=1, keepdims=True)
    var = np.var(x, axis=1, keepdims=True)
    return gamma * (x - mean) / np.sqrt(var + eps) + beta
```

```python
import jax
import jax.numpy as jnp
from jax import lax
from jax.experimental import pallas as pl
from jax.experimental.pallas import tpu as pltpu

EPS = 1e-5
LANES = 128

R = 256
SUB = 128
LAG = 2
WINDOW = 6


def _body(x_hbm, g_ref, b_ref, o_hbm,
          xbuf, obuf, st_loc, st_rem, load_sem, store_sem, send_sem, recv_sem):
    m, n = x_hbm.shape
    nb = m // R
    n_tiles = n // LANES

    my_x = lax.axis_index("x")
    my_y = lax.axis_index("y")
    nbr = (my_x, 1 - my_y)

    def load(i):
        rows = pl.ds(pl.multiple_of(i * R, R), R)
        return pltpu.make_async_copy(x_hbm.at[rows], xbuf.at[rows], load_sem.at[i])

    def store(i):
        rows = pl.ds(pl.multiple_of(i * R, R), R)
        return pltpu.make_async_copy(obuf.at[rows], o_hbm.at[rows], store_sem.at[i])

    def exchange(i):
        return pltpu.make_async_remote_copy(
            src_ref=st_loc.at[i], dst_ref=st_rem.at[i],
            send_sem=send_sem.at[i], recv_sem=recv_sem.at[i],
            device_id=nbr, device_id_type=pl.DeviceIdType.MESH)

    for i in range(WINDOW):
        load(i).start()

    barrier = pltpu.get_barrier_semaphore()
    pl.semaphore_signal(barrier, inc=1, device_id=nbr,
                        device_id_type=pl.DeviceIdType.MESH)

    lane = lax.broadcasted_iota(jnp.int32, (SUB, LANES), 1)

    def stats(i):
        for t in range(R // SUB):
            r0 = pl.multiple_of(i * R + t * SUB, SUB)
            xs = xbuf[pl.ds(r0, SUB), :]
            mean = jnp.sum(xs, axis=1, keepdims=True) * (1.0 / n)
            d = xs - mean
            m2 = jnp.sum(d * d, axis=1, keepdims=True)
            packed = jnp.where(lane == 0, mean, jnp.where(lane == 1, m2, 0.0))
            st_loc[i, :, t * SUB:(t + 1) * SUB] = packed.T[0:8, :]

    def normalise(i):
        loc = st_loc[i]
        rem = st_rem[i]
        mean_a, m2_a = loc[0:1, :], loc[1:2, :]
        mean_b, m2_b = rem[0:1, :], rem[1:2, :]
        delta = mean_a - mean_b
        mean = 0.5 * (mean_a + mean_b)
        m2 = (m2_a + m2_b) + delta * delta * (0.5 * n)
        rstd = lax.rsqrt(m2 * (0.5 / n) + EPS)
        for t in range(R // SUB):
            r0 = pl.multiple_of(i * R + t * SUB, SUB)
            cols = slice(t * SUB, (t + 1) * SUB)
            mean_t = jnp.broadcast_to(mean[:, cols], (LANES, SUB)).T
            rstd_t = jnp.broadcast_to(rstd[:, cols], (LANES, SUB)).T
            for c in range(n_tiles):
                cs = slice(c * LANES, (c + 1) * LANES)
                xs = xbuf[pl.ds(r0, SUB), cs]
                y = (xs - mean_t) * rstd_t * g_ref[:, cs] + b_ref[:, cs]
                obuf[pl.ds(r0, SUB), cs] = y.astype(obuf.dtype)

    def step(i, _):
        @pl.when(i < nb)
        def _():
            load(i).wait()

            @pl.when(i + WINDOW < nb)
            def _():
                load(i + WINDOW).start()

            stats(i)

            @pl.when(i == 0)
            def _():
                pl.semaphore_wait(barrier, 1)

            exchange(i).start()

        @pl.when(i >= LAG)
        def _():
            j = i - LAG
            exchange(j).wait_recv()
            normalise(j)
            store(j).start()

        return None

    lax.fori_loop(0, nb + LAG, step, None)

    def drain(i, _):
        exchange(i).wait_send()
        store(i).wait()
        return None

    lax.fori_loop(0, nb, drain, None)


def pallas_dist_layernorm_xy_m6144_n2048_kernel(
    x: jax.Array,
    gamma: jax.Array,
    beta: jax.Array,
):
    m, n = x.shape
    assert m % R == 0 and R % SUB == 0 and n % LANES == 0
    nb = m // R
    out_dtype = jnp.bfloat16
    return pl.pallas_call(
        _body,
        out_shape=jax.ShapeDtypeStruct((m, n), out_dtype),
        in_specs=[
            pl.BlockSpec(memory_space=pl.ANY),
            pl.BlockSpec(memory_space=pltpu.VMEM),
            pl.BlockSpec(memory_space=pltpu.VMEM),
        ],
        out_specs=pl.BlockSpec(memory_space=pl.ANY),
        scratch_shapes=[
            pltpu.VMEM((m, n), jnp.float32),
            pltpu.VMEM((m, n), out_dtype),
            pltpu.VMEM((nb, 8, R), jnp.float32),
            pltpu.VMEM((nb, 8, R), jnp.float32),
            pltpu.SemaphoreType.DMA((nb,)),
            pltpu.SemaphoreType.DMA((nb,)),
            pltpu.SemaphoreType.DMA((nb,)),
            pltpu.SemaphoreType.DMA((nb,)),
        ],
        compiler_params=pltpu.CompilerParams(
            collective_id=0,
            vmem_limit_bytes=100 * 1024 * 1024,
        ),
    )(x, gamma.reshape(1, n), beta.reshape(1, n))
```

```python
import jax
import jax.numpy as jnp
from jax import lax
from jax.experimental import pallas as pl
from jax.experimental.pallas import tpu as pltpu

EPS = 1e-5
LANES = 128

UNIT = 128
LOAD_UNITS = 2
XCHG_UNITS = 4
TAIL_UNITS = 3
PIECES = (96, 32)
LAG = 5
IN_FLIGHT = 3


def _tree_sum(vals):
    while len(vals) > 1:
        vals = [vals[i] + vals[i + 1] for i in range(0, len(vals), 2)]
    return vals[0]


def _body(x_hbm, gamma_hbm, beta_hbm, o_ref,
          x_vmem, gamma_ref, beta_ref, st_loc, st_rem,
          load_sem, send_sem, recv_sem, gb_sem):
    m, n = x_hbm.shape
    n_tiles = n // LANES
    n_full = m // UNIT - 1
    n_bigu = n_full - TAIL_UNITS
    n_big = n_bigu // LOAD_UNITS
    n_xbig = n_bigu // XCHG_UNITS
    n_piece = len(PIECES)
    assert n_big * LOAD_UNITS == n_bigu and n_xbig * XCHG_UNITS == n_bigu
    assert sum(PIECES) == UNIT and IN_FLIGHT <= n_big and XCHG_UNITS < LAG <= n_full
    piece_row = [n_full * UNIT + sum(PIECES[:v]) for v in range(n_piece)]

    my_x = lax.axis_index("x")
    my_y = lax.axis_index("y")
    neighbour = (my_x, 1 - my_y)

    def load(row0, rows, d):
        rs = pl.ds(row0, rows)
        return pltpu.make_async_copy(
            x_hbm.at[rs], x_vmem.at[rs], load_sem.at[d % IN_FLIGHT])

    def load_big(k):
        rows = LOAD_UNITS * UNIT
        return load(pl.multiple_of(k * rows, rows), rows, k)

    def load_unit(j):
        return load(pl.multiple_of((n_bigu + j) * UNIT, UNIT), UNIT, n_big + j)

    def load_piece(v):
        return load(piece_row[v], PIECES[v], n_big + TAIL_UNITS + v)

    def start_load(d):
        @pl.when(d < n_big)
        def _():
            load_big(d).start()

        @pl.when(jnp.logical_and(d >= n_big, d < n_big + TAIL_UNITS))
        def _():
            load_unit(d - n_big).start()

        for v in range(n_piece):
            @pl.when(d == n_big + TAIL_UNITS + v)
            def _(v=v):
                load_piece(v).start()

    def exchange(t0, nt, sem_idx):
        ts = pl.ds(t0, nt)
        return pltpu.make_async_remote_copy(
            src_ref=st_loc.at[ts], dst_ref=st_rem.at[ts],
            send_sem=send_sem, recv_sem=recv_sem.at[sem_idx],
            device_id=neighbour, device_id_type=pl.DeviceIdType.MESH)

    def exchange_big(k):
        return exchange(k * XCHG_UNITS, XCHG_UNITS, k)

    def exchange_unit(t):
        return exchange(t, 1, t - n_bigu + n_xbig)

    def exchange_piece(v):
        return exchange(n_full + v, 1, n_xbig + TAIL_UNITS + v)

    gamma_copy = pltpu.make_async_copy(gamma_hbm, gamma_ref, gb_sem)
    beta_copy = pltpu.make_async_copy(beta_hbm, beta_ref, gb_sem)
    load_big(0).start()
    gamma_copy.start()
    beta_copy.start()

    barrier = pltpu.get_barrier_semaphore()
    pl.semaphore_signal(barrier, inc=1, device_id=neighbour,
                        device_id_type=pl.DeviceIdType.MESH)

    def stats(t, row0, rows):
        tiles = [x_vmem[pl.ds(row0, rows), c * LANES:(c + 1) * LANES]
                 for c in range(n_tiles)]
        mu = _tree_sum(tiles) * (1.0 / n_tiles)
        sq = _tree_sum([(v - mu) * (v - mu) for v in tiles])
        if rows < UNIT:
            pad = jnp.zeros((UNIT - rows, LANES), jnp.float32)
            mu = jnp.concatenate([mu, pad], axis=0)
            sq = jnp.concatenate([sq, pad], axis=0)
        mu_t = mu.T
        sq_t = sq.T
        mean = jnp.sum(mu_t, axis=0, keepdims=True) * (1.0 / LANES)
        dev = mu_t - mean
        m2 = jnp.sum(sq_t + (dev * dev) * float(n_tiles), axis=0, keepdims=True)
        st_loc[t, 0:1, :] = mean
        st_loc[t, 1:2, :] = m2

    def normalise(t, row0, rows):
        mean_a, m2_a = st_loc[t, 0:1, :], st_loc[t, 1:2, :]
        mean_b, m2_b = st_rem[t, 0:1, :], st_rem[t, 1:2, :]
        delta = mean_a - mean_b
        mean = 0.5 * (mean_a + mean_b)
        m2 = (m2_a + m2_b) + (delta * delta) * (0.5 * n)
        rstd = lax.rsqrt(m2 * (0.5 / n) + EPS)
        mean_t = jnp.broadcast_to(mean, (LANES, UNIT)).T[:rows]
        rstd_t = jnp.broadcast_to(rstd, (LANES, UNIT)).T[:rows]
        for c in range(n_tiles):
            cs = slice(c * LANES, (c + 1) * LANES)
            xs = x_vmem[pl.ds(row0, rows), cs]
            y = (xs - mean_t) * rstd_t * gamma_ref[:, cs] + beta_ref[:, cs]
            o_ref[pl.ds(row0, rows), cs] = y.astype(o_ref.dtype)

    def normalise_unit(j):
        @pl.when(j == 0)
        def _():
            gamma_copy.wait()
            beta_copy.wait()

        @pl.when(jnp.logical_and(j < n_bigu, lax.rem(j, XCHG_UNITS) == 0))
        def _():
            exchange_big(j // XCHG_UNITS).wait_recv()

        @pl.when(j >= n_bigu)
        def _():
            exchange_unit(j).wait_recv()

        normalise(j, pl.multiple_of(j * UNIT, UNIT), UNIT)

    def step(s, carry):
        @pl.when(s == 0)
        def _():
            for d in range(1, IN_FLIGHT):
                load_big(d).start()

        @pl.when(jnp.logical_and(s < n_bigu, lax.rem(s, LOAD_UNITS) == 0))
        def _():
            k = s // LOAD_UNITS
            load_big(k).wait()
            start_load(k + IN_FLIGHT)

        @pl.when(s >= n_bigu)
        def _():
            load_unit(s - n_bigu).wait()
            start_load(s - n_bigu + n_big + IN_FLIGHT)

        stats(s, pl.multiple_of(s * UNIT, UNIT), UNIT)

        @pl.when(s == XCHG_UNITS - 1)
        def _():
            pl.semaphore_wait(barrier, 1)

        @pl.when(jnp.logical_and(s < n_bigu,
                                 lax.rem(s, XCHG_UNITS) == XCHG_UNITS - 1))
        def _():
            exchange_big(s // XCHG_UNITS).start()

        @pl.when(s >= n_bigu)
        def _():
            exchange_unit(s).start()

        @pl.when(s >= LAG)
        def _():
            normalise_unit(s - LAG)

        return carry

    lax.fori_loop(0, n_full, step, 0)

    for v in range(n_piece):
        load_piece(v).wait()
        if v + IN_FLIGHT < n_piece:
            load_piece(v + IN_FLIGHT).start()
        stats(n_full + v, piece_row[v], PIECES[v])
        exchange_piece(v).start()

    def drain(j, carry):
        normalise_unit(j)
        return carry

    lax.fori_loop(n_full - LAG, n_full, drain, 0)

    for v in range(n_piece):
        exchange_piece(v).wait_recv()
        normalise(n_full + v, piece_row[v], PIECES[v])

    pltpu.make_async_copy(st_loc, st_loc, send_sem).wait()


def pallas_dist_layernorm_xy_m6144_n2048_kernel(
    x: jax.Array,
    gamma: jax.Array,
    beta: jax.Array,
):
    m, n = x.shape
    assert m % UNIT == 0 and n % LANES == 0
    n_full = m // UNIT - 1
    n_stat_tiles = n_full + len(PIECES)
    n_exchanges = (n_full - TAIL_UNITS) // XCHG_UNITS + TAIL_UNITS + len(PIECES)
    return pl.pallas_call(
        _body,
        out_shape=pltpu.VMEM((m, n), jnp.bfloat16),
        in_specs=[
            pl.BlockSpec(memory_space=pltpu.HBM),
            pl.BlockSpec(memory_space=pltpu.HBM),
            pl.BlockSpec(memory_space=pltpu.HBM),
        ],
        out_specs=pl.BlockSpec(memory_space=pltpu.VMEM),
        scratch_shapes=[
            pltpu.VMEM((m, n), jnp.float32),
            pltpu.VMEM((1, n), jnp.float32),
            pltpu.VMEM((1, n), jnp.float32),
            pltpu.VMEM((n_stat_tiles, 2, UNIT), jnp.float32),
            pltpu.VMEM((n_stat_tiles, 2, UNIT), jnp.float32),
            pltpu.SemaphoreType.DMA((IN_FLIGHT,)),
            pltpu.SemaphoreType.DMA,
            pltpu.SemaphoreType.DMA((n_exchanges,)),
            pltpu.SemaphoreType.DMA,
        ],
        compiler_params=pltpu.CompilerParams(
            collective_id=0,
            vmem_limit_bytes=64 * 1024 * 1024,
        ),
    )(x, gamma.reshape(1, n), beta.reshape(1, n))
```

```python
import functools

import jax
import jax.numpy as jnp
from jax import lax
from jax.experimental import pallas as pl
from jax.experimental.pallas import tpu as pltpu

EPS = 1e-5
LANES = 128

UNIT = 128
LOAD_UNITS = 2
TAIL_UNITS = 3
PIECES = (96, 32)
IN_FLIGHT = 3
XCHG = (16, 8, 8, 4, 4, 4, 2, 1)
XLAG = 2
NMAX = 2


def _tree_sum(vals):
    while len(vals) > 1:
        vals = [vals[i] + vals[i + 1] for i in range(0, len(vals), 2)]
    return vals[0]


def _body(x_hbm, gamma_hbm, beta_hbm, o_ref,
          x_vmem, gamma_ref, beta_ref, st_loc, st_rem):
    pl.run_scoped(
        functools.partial(_layernorm, x_hbm, gamma_hbm, beta_hbm, o_ref,
                          x_vmem, gamma_ref, beta_ref, st_loc, st_rem),
        pltpu.SemaphoreType.DMA((IN_FLIGHT,)),
        pltpu.SemaphoreType.DMA,
        pltpu.SemaphoreType.DMA,
        pltpu.SemaphoreType.DMA((len(XCHG) + len(PIECES),)),
    )


def _layernorm(x_hbm, gamma_hbm, beta_hbm, o_ref,
               x_vmem, gamma_ref, beta_ref, st_loc, st_rem,
               load_sem, gb_sem, send_sem, recv_sem):
    m, n = x_hbm.shape
    n_tiles = n // LANES
    n_full = m // UNIT - 1
    n_bigu = n_full - TAIL_UNITS
    n_big = n_bigu // LOAD_UNITS
    n_piece = len(PIECES)
    n_xchg = len(XCHG)
    x_first = [sum(XCHG[:b]) for b in range(n_xchg)]
    x_step = [x_first[b] + XCHG[b] - 1 for b in range(n_xchg)]
    piece_row = [n_full * UNIT + sum(PIECES[:v]) for v in range(n_piece)]
    assert n_big * LOAD_UNITS == n_bigu and sum(XCHG) == n_full
    assert sum(PIECES) == UNIT and IN_FLIGHT <= n_big

    my_x = lax.axis_index("x")
    my_y = lax.axis_index("y")
    neighbour = (my_x, 1 - my_y)

    def exchange(t0, nt, sem_idx):
        ts = pl.ds(t0, nt)
        return pltpu.make_async_remote_copy(
            src_ref=st_loc.at[ts], dst_ref=st_rem.at[ts],
            send_sem=send_sem, recv_sem=recv_sem.at[sem_idx],
            device_id=neighbour, device_id_type=pl.DeviceIdType.MESH)

    def exchange_batch(b):
        return exchange(x_first[b], XCHG[b], b)

    def exchange_piece(v):
        return exchange(n_full + v, 1, n_xchg + v)

    def stats(t, row0, rows):
        tiles = [x_vmem[pl.ds(row0, rows), c * LANES:(c + 1) * LANES]
                 for c in range(n_tiles)]
        mu = _tree_sum(tiles) * (1.0 / n_tiles)
        sq = _tree_sum([(v - mu) * (v - mu) for v in tiles])
        if rows < UNIT:
            pad = jnp.zeros((UNIT - rows, LANES), jnp.float32)
            mu = jnp.concatenate([mu, pad], axis=0)
            sq = jnp.concatenate([sq, pad], axis=0)
        mu_t = mu.T
        sq_t = sq.T
        mean = jnp.sum(mu_t, axis=0, keepdims=True) * (1.0 / LANES)
        dev = mu_t - mean
        m2 = jnp.sum(sq_t + (dev * dev) * float(n_tiles), axis=0, keepdims=True)
        st_loc[t, 0:1, :] = mean
        st_loc[t, 1:2, :] = m2

    def normalise(t, row0, rows):
        mean_a, m2_a = st_loc[t, 0:1, :], st_loc[t, 1:2, :]
        mean_b, m2_b = st_rem[t, 0:1, :], st_rem[t, 1:2, :]
        delta = mean_a - mean_b
        mean = 0.5 * (mean_a + mean_b)
        m2 = (m2_a + m2_b) + (delta * delta) * (0.5 * n)
        rstd = lax.rsqrt(m2 * (0.5 / n) + EPS)
        mean_t = jnp.broadcast_to(mean, (LANES, UNIT)).T[:rows]
        rstd_t = jnp.broadcast_to(rstd, (LANES, UNIT)).T[:rows]
        for c in range(n_tiles):
            cs = slice(c * LANES, (c + 1) * LANES)
            xs = x_vmem[pl.ds(row0, rows), cs]
            y = (xs - mean_t) * rstd_t * gamma_ref[:, cs] + beta_ref[:, cs]
            o_ref[pl.ds(row0, rows), cs] = y.astype(o_ref.dtype)

    def normalise_unit(j, carry):
        for b in range(n_xchg):
            @pl.when(j == x_first[b])
            def _(b=b):
                exchange_batch(b).wait_recv()

        normalise(j, pl.multiple_of(j * UNIT, UNIT), UNIT)
        return carry

    def done(s):
        usable = 0
        for b in range(n_xchg):
            usable = usable + jnp.where(s >= x_step[b] + XLAG, XCHG[b], 0)
        return jnp.clip(NMAX * (s - (x_step[0] + XLAG - 1)), 0, usable)

    def load(row0, rows, d):
        rs = pl.ds(row0, rows)
        return pltpu.make_async_copy(
            x_hbm.at[rs], x_vmem.at[rs], load_sem.at[d % IN_FLIGHT])

    def load_big(k):
        rows = LOAD_UNITS * UNIT
        return load(pl.multiple_of(k * rows, rows), rows, k)

    def load_unit(j):
        return load(pl.multiple_of((n_bigu + j) * UNIT, UNIT), UNIT, n_big + j)

    def load_piece(v):
        return load(piece_row[v], PIECES[v], n_big + TAIL_UNITS + v)

    def start_load(d):
        @pl.when(d < n_big)
        def _():
            load_big(d).start()

        @pl.when(jnp.logical_and(d >= n_big, d < n_big + TAIL_UNITS))
        def _():
            load_unit(d - n_big).start()

        for v in range(n_piece):
            @pl.when(d == n_big + TAIL_UNITS + v)
            def _(v=v):
                load_piece(v).start()

    gamma_copy = pltpu.make_async_copy(gamma_hbm, gamma_ref, gb_sem)
    beta_copy = pltpu.make_async_copy(beta_hbm, beta_ref, gb_sem)
    load_big(0).start()
    gamma_copy.start()
    beta_copy.start()

    barrier = pltpu.get_barrier_semaphore()
    pl.semaphore_signal(barrier, inc=1, device_id=neighbour,
                        device_id_type=pl.DeviceIdType.MESH)

    def step(s, carry):
        @pl.when(s == 0)
        def _():
            for d in range(1, IN_FLIGHT):
                load_big(d).start()
            gamma_copy.wait()
            beta_copy.wait()

        @pl.when(jnp.logical_and(s < n_bigu, lax.rem(s, LOAD_UNITS) == 0))
        def _():
            k = s // LOAD_UNITS
            load_big(k).wait()
            start_load(k + IN_FLIGHT)

        @pl.when(s >= n_bigu)
        def _():
            load_unit(s - n_bigu).wait()
            start_load(s - n_bigu + n_big + IN_FLIGHT)

        stats(s, pl.multiple_of(s * UNIT, UNIT), UNIT)

        for b in range(n_xchg):
            @pl.when(s == x_step[b])
            def _(b=b):
                if b == 0:
                    pl.semaphore_wait(barrier, 1)
                exchange_batch(b).start()

        lax.fori_loop(done(s - 1), done(s), normalise_unit, 0)
        return carry

    lax.fori_loop(0, n_full, step, 0)

    for v in range(n_piece):
        load_piece(v).wait()
        if v + IN_FLIGHT < n_piece:
            load_piece(v + IN_FLIGHT).start()
        stats(n_full + v, piece_row[v], PIECES[v])
        exchange_piece(v).start()

    lax.fori_loop(done(n_full - 1), n_full, normalise_unit, 0)

    for v in range(n_piece):
        exchange_piece(v).wait_recv()
        normalise(n_full + v, piece_row[v], PIECES[v])

    pltpu.make_async_copy(st_loc, st_loc, send_sem).wait()


def pallas_dist_layernorm_xy_m6144_n2048_kernel(
    x: jax.Array,
    gamma: jax.Array,
    beta: jax.Array,
):
    m, n = x.shape
    assert m % UNIT == 0 and n % LANES == 0
    n_stat_tiles = m // UNIT - 1 + len(PIECES)
    return pl.pallas_call(
        _body,
        out_shape=pltpu.VMEM((m, n), jnp.bfloat16),
        in_specs=[
            pl.BlockSpec(memory_space=pltpu.HBM),
            pl.BlockSpec(memory_space=pltpu.HBM),
            pl.BlockSpec(memory_space=pltpu.HBM),
        ],
        out_specs=pl.BlockSpec(memory_space=pltpu.VMEM),
        scratch_shapes=[
            pltpu.VMEM((m, n), jnp.float32),
            pltpu.VMEM((1, n), jnp.float32),
            pltpu.VMEM((1, n), jnp.float32),
            pltpu.VMEM((n_stat_tiles, 2, UNIT), jnp.float32),
            pltpu.VMEM((n_stat_tiles, 2, UNIT), jnp.float32),
        ],
        compiler_params=pltpu.CompilerParams(
            collective_id=0,
            vmem_limit_bytes=64 * 1024 * 1024,
        ),
    )(x, gamma.reshape(1, n), beta.reshape(1, n))
```
